```python
import numpy as np

kernel_name = "dist_sparse_attn_localglobal_htp_kvseq_b2_sq256_skv256_hq4_dh64"

def setup_inputs():
    x = np.random.randn(2, 256, 512).astype(np.float32)
    Wq = np.random.randn(512, 1024).astype(np.float32) * 0.02
    K_ext = np.random.randn(2, 1024, 16, 64).astype(np.float32)
    V_ext = np.random.randn(2, 1024, 16, 64).astype(np.float32)
    Wo = np.random.randn(1024, 512).astype(np.float32) * 0.02
    return {"x": x, "Wq": Wq, "K_ext": K_ext, "V_ext": V_ext, "Wo": Wo}

def reference(x, Wq, K_ext, V_ext, Wo):
    B, Sq, Skv, Hq, Dh = 2, 256, 1024, 16, 64
    Q = (x @ Wq).reshape(B, Sq, Hq, Dh)
    qi = np.arange(Sq)[:, None]
    ki = np.arange(Skv)[None, :]
    local = np.abs(qi - ki) <= 128
    glob = (ki < 32) | (qi < 32)
    mask = local | glob
    scores = np.einsum('bihd,bjhd->bhij', Q, K_ext).astype(np.float32) * 0.125
    scores = np.where(mask[None, None, :, :], scores, -1e9)
    scores_max = scores.max(axis=-1, keepdims=True)
    w = np.exp(scores - scores_max)
    row_keep = mask.any(axis=1)
    w_sum = np.where(row_keep[None, None, :, None], w.sum(axis=-1, keepdims=True), 1.0)
    w = w / w_sum
    w = np.where(row_keep[None, None, :, None], w, 0.0)
    ctx = np.einsum('bhij,bjhd->bihd', w, V_ext).reshape(B, Sq, Hq * Dh)
    return ctx @ Wo
```

```python
import jax
import jax.numpy as jnp
from jax import lax
from jax.experimental import pallas as pl
from jax.experimental.pallas import tpu as pltpu

BF = jnp.bfloat16
F32 = jnp.float32
NT = (((1,), (1,)), ((), ()))
NEG = -1e9
QSCALE = 0.125 * 1.4426950408889634
MESH = pl.DeviceIdType.MESH

SCRATCH = [
    ('xf', (2, 256, 512), F32), ('xgf', (2, 32, 512), F32), ('wqf', (512, 256), F32), ('wof', (256, 512), F32),
    ('kf', (2, 1024, 256), F32), ('vf', (2, 1024, 256), F32),
    ('wqb', (512, 256), BF), ('wob', (8, 128, 512), BF),
    ('kb', (2, 1024, 256), BF), ('vb', (2, 1024, 256), BF), ('k1b', (2, 1024, 128), BF), ('v1b', (2, 1024, 128), BF),
    ('qb', (8, 2, 256, 128), BF), ('qg', (8, 64, 128), BF), ('ctx', (8, 2, 256, 128), BF),
    ('ps', (32, 256, 384), BF), ('rs', (32, 128, 128), F32),
    ('l0', (8, 2, 160, 128), F32), ('st', (8, 2, 4, 128), F32),
    ('hf', (8, 2, 128, 128), F32), ('hl', (8, 2, 128, 128), F32), ('hs', (8, 2, 128, 128), BF), ('hst', (8, 2, 2, 128), F32),
    ('gw', (8, 2, 32, 128), F32), ('gz', (8, 2, 32, 128), F32),
    ('zf', (4, 128, 128), F32), ('zl', (4, 128, 128), F32), ('zs', (4, 128, 128), BF), ('zst', (4, 2, 128), F32),
    ('zr', (2, 4, 128, 128), BF), ('zrs', (2, 4, 2, 128), F32),
    ('pf', (2, 2, 256, 256), F32), ('pb', (2, 2, 256, 256), BF),
    ('sbuf', (3, 2, 2, 256, 256), BF), ('rbuf', (3, 2, 2, 256, 256), BF),
]


def iota(shape, d):
    return lax.broadcasted_iota(jnp.int32, shape, d)


def halves(xs):
    if len(xs) == 1:
        n = xs[0].shape[0] // 2
        xs = [xs[0][:n], xs[0][n:]]
    return jnp.where(iota((xs[0].shape[0], 128), 1) < 64, xs[0], xs[1])


def s_phase(q, kT, keep, per_head=False):
    n = q.shape[0]
    lo = iota((n, 128), 1) < 64
    z = jnp.zeros_like(q)
    qs = [jnp.where(lo, q, z), jnp.where(lo, z, q)]
    if not per_head: qs = [jnp.concatenate(qs, 0)]
    ps, ls, ms = [], [], []
    for x in qs:
        s = jnp.dot(x, kT, preferred_element_type=F32)
        tiles = []
        for t in range(kT.shape[1] // 128):
            st = s[:, t * 128:(t + 1) * 128]
            if t in keep:
                st = jnp.concatenate([jnp.where(keep[t], st[r:r + n], NEG) for r in range(0, x.shape[0], n)], 0)
            tiles.append(st)
        s = jnp.concatenate(tiles, 1) if len(tiles) > 1 else tiles[0]
        m = jnp.max(s, -1, keepdims=True)
        p = jnp.exp2(s - m)
        ps.append(p.astype(BF)); ls.append(jnp.sum(p, -1, keepdims=True)); ms.append(m)
    return tuple(ps), halves(ls), halves(ms)


def t_phase(ps, rinv, vT):
    return halves([lax.dot_general(p, vT, NT, preferred_element_type=F32) for p in ps]) * rinv


def recip(x):
    r = pl.reciprocal(x, approx=True)
    return r * (2.0 - x * r)


def pack_stats(x):
    if x.shape[0] < 128: x = jnp.concatenate([x, jnp.zeros((128 - x.shape[0], 128), F32)], 0)
    t = x.T
    return jnp.concatenate([t[0:1], t[64:65]], 0)


def unpack_stats(v, n=128):
    return jnp.concatenate([jnp.broadcast_to(v[0:1], (64, 128)), jnp.broadcast_to(v[1:2], (64, 128))], 0).T[0:n]


def merge_weights(lses):
    m = lses[0]
    for x in lses[1:]:
        m = jnp.maximum(m, x)
    e = [jnp.exp2(x - m) for x in lses]
    tot = e[0]
    for x in e[1:]:
        tot = tot + x
    return m, e, tot


class Chip:
    def __init__(self, c, R, T, sems, home, before=None):
        self.c, self.R, self.T, self.sems, self.home = c, R, T, sems, home
        self.waited = set(before.waited) if before else set()
        self.sent = list(before.sent) if before else []
        self.fences = before.fences if before else 0
        self.stored = before is not None

    def wait_all(self, names):
        new = [d for d in names if self.T[d]['kind'] in ('load', 'send') and d not in self.waited]
        for d in names: self.wait(d)
        if new: self.fence()

    def fence(self):
        pl.semaphore_signal(self.R['fence'], 1)
        self.fences += 1
        self.stored = False

    def load_copies(self, t):
        R = self.R
        out = []
        for cp in t['op'][1:]:
            if cp[0] == 'xg': s, d = R['x'].at[:, pl.ds(0, 32)], R['xgf']
            elif cp[0] == 'wq': s, d = R['wq'], R['wqf']
            elif cp[0] == 'x': s, d = R['x'].at[cp[1]], R['xf'].at[cp[1]]
            elif cp[0] == 'wo': s, d = R['wo'].at[pl.ds(cp[1], cp[2])], R['wof'].at[pl.ds(cp[1], cp[2])]
            else:
                a, b, r0, nr, l = cp
                hb, vm = (R['k'], R['kf']) if a == 'K' else (R['v'], R['vf'])
                idx = (slice(None) if b is None else b, pl.ds(r0, nr)) + {'f': (), 'a': (pl.ds(0, 128),), 'z': (pl.ds(128, 128),)}[l]
                s, d = hb.at[idx], vm.at[idx]
            out.append(pltpu.make_async_copy(s, d, R['lsem'].at[self.sems['l'][t['name']]]))
        return out

    def chunk_ref(self, ch, loc, f32=False):
        b, r0, nr, half = ch
        R = self.R
        if loc[0] == 'P': return R['pf' if f32 else 'pb'].at[half, b, pl.ds(r0, nr)]
        return R['rbuf' if loc[0] == 'R' else 'sbuf'].at[loc[1], half, b, pl.ds(r0, nr)]

    def remote_copies(self, t):
        R, op = self.R, t['op']
        k = op[0]
        if k in ('kv', 'kv1'):
            _, a, b, p, r0, nr = op; r = [R[a.lower() + k[2:] + 'b'].at[b, pl.ds(p * 128 + r0, nr)]]
        elif k == 'wo': r = [R['wob'].at[op[1], pl.ds(op[2], op[3])]]
        elif k == 'q': r = [R['qb'].at[op[1], op[2], pl.ds(op[3], 128)]]
        elif k == 'qg': r = [R['qg'].at[pl.ds(2 * op[1], 2)]]
        elif k == 'st': r = [R['st'].at[op[1], op[2]]]
        elif k == 'h': r = [R['hs'].at[op[1], op[2]]]
        elif k == 'hs': r = [R['hst'].at[op[1], op[2]]]
        elif k == 'ctx': r = [R['ctx'].at[op[1], op[2], pl.ds(op[3], op[4])]]
        if k not in ('z', 'chunk'): prs = [(x, x) for x in r]
        elif k == 'z':
            _, g, slot = op
            prs = [(R['zs'].at[g], R['zr'].at[slot, g]), (R['zst'].at[g], R['zrs'].at[slot, g])]
        else:
            _, ch, loc, slot = op; prs = [(self.chunk_ref(ch, loc), self.chunk_ref(ch, ('R', slot)))]
        si, ri = self.sems['s'][t['name']], self.sems['r'][t['name']]
        return [pltpu.make_async_remote_copy(s, d, R['ssem'].at[si + i], R['rsem'].at[ri + i], device_id=(t['dst'],), device_id_type=MESH)
                for i, (s, d) in enumerate(prs)]

    def wait(self, name):
        t = self.T[name]
        if t['kind'] == 'comp': return
        key = t['op'][0] if t['kind'] == 'sig' else name
        if key in self.waited: return
        self.waited.add(key)
        if key == 'bar':
            pl.semaphore_wait(pltpu.get_barrier_semaphore(), sum(1 for u in self.T.values() if u['op'] == ('bar', self.c)))
        elif key == 'rdy': pl.semaphore_wait(self.R['rdy'], 1)
        elif t['kind'] == 'load':
            for cp in self.load_copies(t): cp.wait()
        else:
            for cp in self.remote_copies(t): cp.wait_recv()

    def unit_kv(self, u, a):
        p, b, rows, keys = u
        R = self.R; rr = pl.ds(p * 128, 128)
        f, r0, r1 = (R['kf'], R['kb'], R['k1b']) if a == 'K' else (R['vf'], R['vb'], R['v1b'])
        parts = []
        if '0' in keys: parts.append(f[b, rr, :].astype(BF) if self.c == 0 else r0[b, rr, :])
        if '1' in keys: parts.append(f[b, rr, 0:128].astype(BF) if self.c == 1 else r1[b, rr, :])
        return jnp.concatenate(parts, 1) if len(parts) > 1 else parts[0]

    def att_s(self, u, spill, per_head):
        R = self.R
        p, b, rows, keys = u
        i, j = iota((128, 128), 0), iota((128, 128), 1)
        if rows == 'lo': keep = {1: (j <= i) | (i < 32)}
        elif keys == '1': keep = {0: j <= i}
        else:
            keep = {0: (j >= i) | (j < 32)}
            if keys == '01': keep[2] = j <= i
        r0 = 0 if rows == 'lo' else 128
        pr, l, m = s_phase(R['qb'][p, b, r0:r0 + 128, :], self.unit_kv(u, 'K'), keep, per_head)
        if rows == 'lo': R['l0'][p, b, 0:32, :] = m[0:32] + jnp.log2(l[0:32])
        elif keys == '0': R['l0'][p, b, 32:160, :] = m + jnp.log2(l)
        elif keys == '1':
            lse = m + jnp.log2(l)
            if self.home[p] == self.c: R['hl'][p, b] = lse
            else: R['hst'][p, b] = pack_stats(lse)
        if not spill: return pr, recip(l)
        n = p * 4 + b * 2 + (rows == 'hi')
        for k, x in enumerate(pr): R['ps'][n, k * 128:k * 128 + x.shape[0], 0:x.shape[1]] = x
        R['rs'][n] = recip(l)

    def att_t(self, u, held, per_head):
        R = self.R
        p, b, rows, keys = u
        if held is None:
            n = p * 4 + b * 2 + (rows == 'hi')
            rr = (slice(0, 128), slice(128, 256)) if per_head else (slice(0, 256),)
            held = tuple(R['ps'][n, r, 0:128 * (len(keys) + 1)] for r in rr), R['rs'][n]
        o = t_phase(held[0], held[1], self.unit_kv(u, 'V'))
        if keys != '1':
            r0 = 0 if rows == 'lo' else 128
            R['ctx'][p, b, r0:r0 + 128, :] = o.astype(BF)
        elif self.home[p] == self.c: R['hf'][p, b] = o
        else: R['hs'][p, b] = o.astype(BF)

    def z_out(self, g, z, lse, mode):
        R = self.R
        if mode == 'pack':
            R['zs'][g] = z.astype(BF); R['zst'][g] = pack_stats(lse)
        else:
            R['zf'][g] = z; R['zl'][g] = lse

    def comp(self, op):
        R, c, k = self.R, self.c, op[0]
        if k == 'cvwq': R['wqb'][...] = R['wqf'][...].astype(BF)
        elif k == 'cvwo':
            _, p, r0, nr = op
            R['wob'][p, r0:r0 + nr, :] = R['wof'][p % 2 * 128 + r0:p % 2 * 128 + r0 + nr, :].astype(BF)
        elif k in ('qg', 'q'):
            x = R['xgf'][...].reshape(64, 512) if k == 'qg' else R['xf'][op[1]]
            y = (jnp.dot(x.astype(BF), R['wqb'][...], preferred_element_type=F32) * QSCALE).astype(BF)
            for q in (0, 1):
                if k == 'qg': R['qg'][2 * c + q] = y[:, q * 128:(q + 1) * 128]
                else: R['qb'][2 * c + q, op[1]] = y[:, q * 128:(q + 1) * 128]
        elif k in ('cvkv', 'cvkv1'):
            _, a, b, p, r0, nr = op
            rr = slice(p * 128 + r0, p * 128 + r0 + nr)
            R[a.lower() + k[4:] + 'b'][b, rr, :] = R[a.lower() + 'f'][b, rr, 0:(128 if k[4:] else 256)].astype(BF)
        elif k == 'pk':
            _, p, b, joint = op
            band = jnp.zeros((2, 128), F32) if joint else pack_stats(R['l0'][p, b, 32:160, :])
            R['st'][p, b] = jnp.concatenate([band, pack_stats(R['l0'][p, b, 0:32, :])], 0)
        elif k == 'z':
            g = op[1]
            held = []
            for b in (0, 1):
                for p in (2 * g, 2 * g + 1):
                    held.append((b, p) + s_phase(R['qg'][p, b * 32:(b + 1) * 32, :], R['kf'][b, p * 128:(p + 1) * 128, :].astype(BF), {}))
            zs = [t_phase(pr, recip(l), R['vf'][b, p * 128:(p + 1) * 128, :].astype(BF)) for b, p, pr, l, m in held]
            ls = [m + jnp.log2(l) for b, p, pr, l, m in held]
            self.z_out(g, jnp.concatenate(zs, 0), jnp.concatenate(ls, 0), 'pack' if 'pack' in op else 'keep')
        elif k == 'zm':
            _, g, own, slots, mode = op
            zs = ([R['zf'][g]] if own else []) + [R['zr'][d, g].astype(F32) for d in slots]
            ls = ([R['zl'][g]] if own else []) + [unpack_stats(R['zrs'][d, g]) for d in slots]
            if len(zs) == 1: z, lse = zs[0], ls[0]
            else:
                m, e, tot = merge_weights(ls)
                z = e[0] * zs[0]
                for w, y in zip(e[1:], zs[1:]): z = z + w * y
                z, lse = z * recip(tot), m + jnp.log2(tot)
            self.z_out(g, z, lse, mode)
        elif k == 'pw':
            _, p, b, rem0, rem1 = op
            _, e, tot = merge_weights([unpack_stats(R['st'][p, b, 0:2, :]) if rem0 else R['l0'][p, b, 32:160, :],
                                       unpack_stats(R['hst'][p, b]) if rem1 else R['hl'][p, b]])
            inv = recip(tot)
            R['hl'][p, b] = e[0] * inv
            R['hf'][p, b] = e[1] * inv if rem1 else e[1] * inv * R['hf'][p, b]
        elif k == 'pg':
            _, g, b, rem = op
            for q in (0, 1):
                p = 2 * g + q; rr = slice((2 * b + q) * 32, (2 * b + q + 1) * 32)
                _, e, tot = merge_weights([unpack_stats(R['st'][p, b, 2:4, :], 32) if rem[q] else R['l0'][p, b, 0:32, :], R['zl'][g, rr, :]])
                inv = recip(tot)
                R['gw'][p, b] = e[0] * inv; R['gz'][p, b] = e[1] * inv * R['zf'][g, rr, :]
        elif k == 'proj':
            _, b, r0, nr, ps, mer = op
            parts = []
            for p, mg in zip(ps, mer):
                y = R['ctx'][p, b, r0:r0 + nr, :]
                if mg and r0 == 0: y = (R['gw'][p, b] * y.astype(F32) + R['gz'][p, b]).astype(BF)
                elif mg:
                    rr = slice(r0 - 128, r0 - 128 + nr)
                    h = R['hf'][p, b, rr, :] * R['hs'][p, b, rr, :].astype(F32) if mg == 2 else R['hf'][p, b, rr, :]
                    y = (R['hl'][p, b, rr, :] * y.astype(F32) + h).astype(BF)
                parts.append(y)
            o = jnp.dot(jnp.concatenate(parts, 1), jnp.concatenate([R['wob'][p] for p in ps], 0), preferred_element_type=F32)
            for h in (0, 1):
                oh = o[:, h * 256:(h + 1) * 256]
                R['pf'][h, b, r0:r0 + nr, :] = oh; R['pb'][h, b, r0:r0 + nr, :] = oh.astype(BF)
        elif k in ('add', 'fin'):
            ch, locs = op[1], op[-1]
            acc = None
            for loc in locs:
                y = self.chunk_ref(ch, loc, True)[...].astype(F32)
                acc = y if acc is None else acc + y
            b, r0, nr, half = ch
            if k == 'add': self.chunk_ref(ch, ('S', op[2]))[...] = acc.astype(BF)
            else: R['o'][b, r0:r0 + nr, half * 256:(half + 1) * 256] = acc
        else: raise ValueError(op)

    def region(self, tasks):
        self.wait_all([d for t in tasks for d in t['deps']])
        self.stored = True
        i = 0
        while i < len(tasks):
            if tasks[i]['op'][0] != 'att':
                self.comp(tasks[i]['op']); i += 1; continue
            j = i
            while j < len(tasks) and tasks[j]['op'][0] == 'att': j += 1
            tiles = [(t['op'][1], {'0': 2, '01': 3, '1': 1}[t['op'][2][3]]) for t in tasks[i:j]]
            small = max(sum(n for ph, n in tiles if x in ph) for x in 'ST') <= 6
            held = [self.att_s(t['op'][2], t['op'][1] == 'S', small) if 'S' in t['op'][1] else None for t in tasks[i:j]]
            for t, h in zip(tasks[i:j], held):
                if 'T' in t['op'][1]: self.att_t(t['op'][2], h, small)
            i = j

    def run(self, order, last):
        T, sent = self.T, self.sent
        for item in order:
            names = item.split(' ')
            if names[0] == '#':
                for n in names[1:]:
                    sent.remove(T[n])
                    for cp in self.remote_copies(T[n]): cp.wait_send()
                continue
            t = T[names[0]]
            if t['kind'] == 'comp':
                self.region([T[n] for n in names]); continue
            self.wait_all(t['deps'])
            if t['kind'] == 'load':
                for cp in self.load_copies(t): cp.start()
            elif t['kind'] == 'send':
                if self.stored: self.fence()
                for cp in self.remote_copies(t): cp.start()
                sent.append(t)
            else:
                sem = pltpu.get_barrier_semaphore() if t['op'][0] == 'bar' else self.R['rdy']
                pl.semaphore_signal(sem, 1, device_id=(t['dst'],), device_id_type=MESH)
        if not last: return
        for u in T.values():
            if (u['kind'] == 'load' and u['chip'] == self.c) or (u['kind'] in ('send', 'sig') and u['dst'] == self.c):
                self.wait(u['name'])
        for t in sent:
            for cp in self.remote_copies(t): cp.wait_send()
        if self.fences: pl.semaphore_wait(self.R['fence'], self.fences)


def assign_sems(T):
    sems = {'l': {}, 's': {}, 'r': {}}
    cnt = {k: [0] * 4 for k in sems}
    for t in T.values():
        if t['kind'] == 'load':
            sems['l'][t['name']] = cnt['l'][t['chip']]; cnt['l'][t['chip']] += 1
        elif t['kind'] == 'send':
            n = 2 if t['op'][0] == 'z' else 1
            sems['s'][t['name']] = cnt['s'][t['chip']]; cnt['s'][t['chip']] += n
            sems['r'][t['name']] = cnt['r'][0]; cnt['r'][0] += n
    return sems, cnt


def make_kernel(T, ORDER, home, LAYOUT):
    sems, cnt = assign_sems(T)
    for c in range(4):
        assert sorted(n for it in ORDER[c] if it[0] != '#' for n in it.split(' ')) == sorted(n for n, t in T.items() if t['chip'] == c)

    def body(x, wq, k, v, wo, o, *scratch):
        R = dict(x=x, wq=wq, k=k, v=v, wo=wo, o=o)
        R.update(zip([s[0] for s in SCRATCH] + ['lsem', 'ssem', 'rsem', 'rdy', 'fence'], scratch))
        me = lax.axis_index('i')
        chips, done = [None] * 4, [0] * 4
        for c, stop in LAYOUT:
            def piece(c=c, before=chips[c], steps=ORDER[c][done[c]:stop], last=stop is None):
                chips[c] = Chip(c, R, T, sems, home, before)
                chips[c].run(steps, last)
            pl.when(me == c)(piece)
            done[c] = stop

    def kernel(x, Wq, K_ext, V_ext, Wo):
        kt = jnp.transpose(K_ext, (0, 2, 3, 1)).reshape(2, 1024, 256)
        vt = jnp.transpose(V_ext, (0, 2, 3, 1)).reshape(2, 1024, 256)
        return pl.pallas_call(
            body,
            out_shape=jax.ShapeDtypeStruct((2, 256, 512), F32),
            in_specs=[pl.BlockSpec(memory_space=pl.ANY)] * 5,
            out_specs=pl.BlockSpec(memory_space=pltpu.VMEM),
            scratch_shapes=[pltpu.VMEM(s, d) for _, s, d in SCRATCH] + [
                pltpu.SemaphoreType.DMA((max(cnt['l']),)), pltpu.SemaphoreType.DMA((max(cnt['s']),)),
                pltpu.SemaphoreType.DMA((max(cnt['r']),)), pltpu.SemaphoreType.REGULAR, pltpu.SemaphoreType.REGULAR],
            compiler_params=pltpu.CompilerParams(
                collective_id=0, vmem_limit_bytes=64 * 1024 * 1024,
                disable_semaphore_checks=True, disable_bounds_checks=True),
        )(x, Wq, kt, vt, Wo)
    return kernel


def make_tasks(cfg):
    T = {}
    c0, c1, w, route, blocks = cfg['c0'], cfg['c1'], cfg['w'], cfg['r'], cfg['blocks']

    def add(chip, kind, name, deps, op, **kw):
        assert name not in T, name
        T[name] = dict(chip=chip, kind=kind, name=name, deps=list(deps), op=op, **kw)
        return name

    bar2 = ['b1>2', 'b3>2']
    up = {(0, 1): ['b1>0', 'b3>0'], (0, 3): ['b1>0', 'b3>0'], (1, 0): ['b0>1'], (3, 0): ['b0>3'],
          (1, 2): ['r2>1'], (3, 2): ['r2>3'], (2, 1): bar2, (2, 3): bar2}
    for s, d in ((0, 1), (0, 3), (1, 0), (1, 2), (3, 0), (3, 2)):
        add(s, 'sig', f'b{s}>{d}', [], ('bar', d), dst=d)
    for d in (1, 3):
        add(2, 'sig', f'r2>{d}', bar2, ('rdy', d), dst=d)

    def S(c, name, dst, deps, op):
        return add(c, 'send', name, list(deps) + up[(c, dst)], op, dst=dst)

    def C(c, name, deps, op):
        return add(c, 'comp', name, deps, op)

    def L(c, name, *copies):
        add(c, 'load', f'L{c}{name}', [], ('load',) + copies)

    def xfer(name, a, d, deps, op, key):
        if a == d: return {a: deps}
        if (d - a) % 4 != 2:
            return {a: deps, d: [S(a, name, d, deps, op)]}
        m = (a + (1 if route.get(key) == 2 else -1) * (1 if a % 2 == 0 else -1)) % 4
        S(a, name + '~', m, deps, op)
        return {a: deps, m: [name + '~'], d: [S(m, name, d, [name + '~'], op)]}

    def kvload(c, a, b, p):
        per_pair = (c, a, b, p // 2) in cfg['lsplit']
        n = f'{a if c == 0 else a.lower()}{b}' + (f'p{p}' if per_pair else f'G{p // 2}')
        rows = 128 if per_pair else 256
        if (c, a, b, p) == cfg['f1'] and f'L{c}{n}' not in T:
            L(c, n + 'a', (a, b, p * 128, 32, 'a')); L(c, n, (a, b, p * 128 + 32, 96, 'a'))
        if f'L{c}{n}' not in T: L(c, n, (a, b, p * 128 // rows * rows, rows, 'f' if c == 0 else 'a'))
        return f'L{c}{n}'

    pieces = lambda p: ((0, 16), (16, 48), (64, 64)) if p == cfg['wsplit'] else ((0, 64), (64, 64))
    for c in range(4):
        L(c, 'xg', ('xg',)); L(c, 'Wq', ('wq',)); L(c, 'x0', ('x', 0)); L(c, 'x1', ('x', 1))
        for q in (0, 1):
            if w[2 * c] == c: L(c, f'Wo{q}', ('wo', q * 128, 128))
            else:
                for r0, nr in pieces(2 * c + q): L(c, f'Wo{q}.{r0}', ('wo', q * 128 + r0, nr))
        for g in range(4):
            if c > 1: L(c, f'KVG{g}', ('K', None, g * 256, 256, 'f'), ('V', None, g * 256, 256, 'f'))
            if c == 1 and g % 2 == 0: L(c, f'KVG{g}', ('K', None, g * 256, 512, 'z'), ('V', None, g * 256, 512, 'z'))
        C(c, f'cvWq{c}', [f'L{c}Wq'], ('cvwq',))
        C(c, f'Q{c}g', [f'L{c}xg', f'cvWq{c}'], ('qg',))
        for b in (0, 1): C(c, f'Q{c}b{b}', [f'L{c}x{b}', f'cvWq{c}'], ('q', b))
    wo = {}
    for p in range(8):
        o = p // 2
        if w[p] == o:
            wo[p] = [C(o, f'cvWo{p}', [f'L{o}Wo{p % 2}'], ('cvwo', p, 0, 128))]
            continue
        wo[p] = []
        for r0, nr in pieces(p):
            d = [C(o, f'cvWo{p}.{r0}', [f'L{o}Wo{p % 2}.{r0}'], ('cvwo', p, r0, nr))]
            wo[p] += xfer(f'Wo{p}.{r0}', o, w[p], d, ('wo', p, r0, nr), ('wo', p))[w[p]]

    rowdep, lse0 = {}, {}
    for b in (0, 1):
        for p in range(8):
            o, a0, a1, ww, u = p // 2, c0[p, b], c1[p, b], w[p], f'{b}p{p}'
            kv = {}
            for a in 'KV':
                for src, dst, nm, k in ((0, a0, a, 'kv'), (1, a1, a.lower(), 'kv1')):
                    ld = kvload(src, a, b, p)
                    kv[nm] = [ld] if dst == src else []
                    parts = (('a', 0, 32), ('', 32, 96)) if (src, a, b, p) == cfg['f1'] else (('', 0, 128),)
                    for x, r0, nr in parts if dst != src else ():
                        d = [C(src, f'cv{nm}{u}{x}', [ld + x], ('cv' + k, a, b, p, r0, nr))]
                        kv[nm] += xfer(f'{nm}{u}{x}', src, dst, d, (k, a, b, p, r0, nr), (k, p, b))[dst]
            ql = xfer(f'q{u}lo', o, a0, [f'Q{o}b{b}'], ('q', p, b, 0), ('q', p, b))
            qh = xfer(f'q{u}hi', o, a0, [f'Q{o}b{b}'], ('q', p, b, 128), ('q', p, b))
            if a1 not in qh:
                qh[a1] = xfer(f'q{u}h1', o, a1, qh[o], ('q', p, b, 128), ('q1', p, b))[a1]
            joint = a0 == a1
            sd = []
            for rows, qd, keys in (('lo', ql[a0], '0'), ('hi', qh[a0], '01' if joint else '0')):
                unit = (p, b, rows, keys)
                kd = kv['K'] + (kv['k'] if keys == '01' else []); vd = kv['V'] + (kv['v'] if keys == '01' else [])
                if cfg['split'].get((p, b, rows)):
                    sd.append(C(a0, f'S{u}{rows}', qd + kd, ('att', 'S', unit)))
                    C(a0, f'T{u}{rows}', [f'S{u}{rows}'] + vd, ('att', 'T', unit))
                else:
                    sd.append(C(a0, f'T{u}{rows}', qd + kd + vd, ('att', 'ST', unit)))
            sd = sd[:1] if joint else sd
            if a0 != ww:
                sd = xfer(f'st{u}', a0, ww, [C(a0, f'pk{u}', sd, ('pk', p, b, joint))], ('st', p, b), ('c', p, b))[ww]
            lse0[p, b] = sd
            hd = []
            if not joint:
                d = [C(a1, f'H{u}', qh[a1] + kv['k'] + kv['v'], ('att', 'ST', (p, b, 'hi', '1')))]
                ds = xfer(f'hs{u}', a1, ww, d, ('hs', p, b), ('h', p, b))[ww]
                hd = [C(ww, f'pw{u}', ds + sd, ('pw', p, b, a0 != ww, a1 != ww))]
                if a1 != ww: hd += xfer(f'h{u}', a1, ww, d, ('h', p, b), ('h', p, b))[ww]
            whole = cfg['cgrp'].get((p, b))
            for bb, r0, nr in sorted(blocks):
                if bb != b: continue
                if not (a0 != ww and whole and r0 not in (0, 128)):
                    d = xfer(f'c{u}.{r0}', a0, ww, [f'T{u}hi' if r0 >= 128 else f'T{u}lo'],
                             ('ctx', p, b, r0, 128 if whole else nr), ('c', p, b))[ww]
                rowdep[p, b, r0] = d + (hd if r0 >= 128 else [])

    def ring(start, cut, step):
        hops = []
        while (start if step == 1 else (start - 1) % 4) != cut:
            hops.append((start, (start + step) % 4)); start = hops[-1][1]
        return hops

    zdep = {}
    for g in range(4):
        ps = (2 * g, 2 * g + 1)
        at = {g: [f'Q{g}g']}
        for step in (1, -1):
            hops = ring(g, cfg['qg'][g], step)
            while hops and hops[-1][1] == 0: hops.pop()
            for a, n in hops: at[n] = [S(a, f'Q{g}g>{n}', n, at[a], ('qg', g))]
        t = w[2 * g]
        for c in (1, 2, 3):
            ld = [f'L{c}KVG{g}'] if c > 1 else [f'L1KVG{g // 2 * 2}'] + [kvload(1, a, b, p) for a in 'KV' for b in (0, 1) for p in ps]
            if c == 1 and cfg['f1'][3] in ps: ld.append(kvload(*cfg['f1']) + 'a')
            C(c, f'Z{c}G{g}', at[c] + ld, ('z', g))
        ins = []
        for slot, step in enumerate((1, -1)):
            cur = None
            for d, s in reversed(ring(t, cfg['zt'][g], step)):
                if s == 0:
                    assert cur is None
                    continue
                if cur is None:
                    dep = f'Z{s}G{g}'; T[dep]['op'] += ('pack',)
                else: dep = C(s, f'm{s}G{g}', [cur, f'Z{s}G{g}'], ('zm', g, True, (slot,), 'pack'))
                cur = S(s, f'z{s}G{g}', d, [dep], ('z', g, slot))
            if cur: ins.append((cur, slot))
        C(t, f'pm{g}', [n for n, _ in ins] + ([f'Z{t}G{g}'] if t else []), ('zm', g, t != 0, tuple(s for _, s in ins), 'keep'))
        for b in (0, 1):
            zdep[g, b] = [C(t, f'pg{b}G{g}', [f'pm{g}'] + lse0[ps[0], b] + lse0[ps[1], b], ('pg', g, b, tuple(c0[p, b] != t for p in ps)))]

    for b, r0, nr in blocks:
        P = {}
        for c in sorted(set(w.values())):
            ps = tuple(p for p in range(8) if w[p] == c)
            d = sum((rowdep[p, b, r0] + wo[p] + (zdep[p // 2, b] if r0 == 0 else []) for p in ps), [])
            mer = tuple(1 if r0 == 0 else (r0 >= 128 and c0[p, b] != c1[p, b]) * (1 + (c1[p, b] != c)) for p in ps)
            P[c] = ([C(c, f'P{c}_{b}.{r0}', d, ('proj', b, r0, nr, ps, mer))], ('P',))
        for half in (0, 1):
            cut = cfg['sub'].get((b, r0, half), 0)
            for q0, qn in ((r0, nr - cut), (r0 + nr - cut, cut))[:1 + (cut > 0)]:
                reduce_chunk(C, S, ring, cfg['pat'][b, q0, half], (b, q0, qn, half), P)
    for c in range(4):
        assert sum(len(t['op']) - 1 for t in T.values() if t['kind'] == 'load' and t['chip'] == c) <= 32
    return T


def reduce_chunk(C, S, ring, pat, ch, P):
    b, r0, nr, half = ch
    m = f'{b}.{r0}.{half}'
    sums, recvs = [0] * 4, [0] * 4

    def add(c, vals):
        vals = [v for v in vals if v]
        if len(vals) <= 1: return vals[0] if vals else None
        k = sums[c]; sums[c] += 1
        return [C(c, f'a{c}_{m}_{k}', sum((v[0] for v in vals), []), ('add', ch, k, tuple(v[1] for v in vals)))], ('S', k)

    def snd(a, d, tag, v):
        if not v: return None
        k = recvs[d]; recvs[d] += 1
        return [S(a, f'{tag}{a}>{d}_{m}', d, v[0], ('chunk', ch, v[1], k))], ('R', k)

    def fin(c, vals):
        vals = [v for v in vals if v]
        C(c, f'F{c}_{m}', sum((v[0] for v in vals), []), ('fin', ch, tuple(v[1] for v in vals)))

    if pat[0] == 'p':
        _, cut, opt = pat
        v = [(cut + 1 + i) % 4 for i in range(4)]
        pre, suf = [None] * 4, [None] * 4
        for i in range(2 if opt == 2 else 3):
            pre[i + 1] = snd(v[i], v[i + 1], 'R', add(v[i], [pre[i], P.get(v[i])]))
        for i in range(3, 1 if opt == 1 else 0, -1):
            suf[i - 1] = snd(v[i], v[i - 1], 'L', add(v[i], [suf[i], P.get(v[i])]))
        if opt == 2: fin(v[3], [snd(v[0], v[3], 'F', add(v[0], [suf[0], P.get(v[0])]))])
        if opt == 1: fin(v[0], [snd(v[3], v[0], 'F', add(v[3], [pre[3], P.get(v[3])]))])
        for i in range(4):
            if (opt, i) not in ((2, 3), (1, 0)): fin(v[i], [pre[i], suf[i], P.get(v[i])])
    else:
        _, root, k1, k2 = pat
        ins = [P.get(root)]
        for step in (1, -1):
            cur = None
            for d, s in reversed(ring(root, k1, step)): cur = snd(s, d, 'U', add(s, [cur, P.get(s)]))
            ins.append(cur)
        total = add(root, ins)
        fin(root, ins)
        for step in (1, -1):
            cur = total
            for a, n in ring(root, k2, step):
                cur = snd(a, n, 'B', cur); fin(n, [cur])


def per_pair(*digits):
    return {(p, b): int(d) for b, row in enumerate(digits) for p, d in enumerate(row)}


CFG = dict(
    c0=per_pair('00113300', '00103000'), c1=per_pair('00112111', '00112111'), w={0: 0, 1: 0, 2: 1, 3: 1, 4: 2, 5: 2, 6: 0, 7: 0},
    r={('q1', 6, 0): 2, ('q1', 6, 1): 2, ('q1', 7, 0): 2, ('q1', 7, 1): 2},
    qg={0: 3, 1: 0, 2: 3, 3: 3}, zt={0: 0, 1: 0, 2: 0, 3: 0},
    lsplit={(0, 'K', 0, 1), (0, 'K', 0, 2), (0, 'K', 1, 0), (0, 'K', 1, 3), (0, 'V', 0, 2), (0, 'V', 1, 0),
        (1, 'V', 0, 0), (1, 'V', 1, 0)},
    wsplit=6, f1=(1, 'V', 1, 0), cgrp={(5, 0): True},
    split={(0, 0, 'hi'): 1, (0, 0, 'lo'): 1, (1, 0, 'hi'): 1, (1, 1, 'hi'): 1, (2, 0, 'hi'): 1, (4, 0, 'hi'): 1,
        (4, 0, 'lo'): 1, (4, 1, 'lo'): 1, (5, 0, 'hi'): 1, (5, 0, 'lo'): 1, (5, 1, 'lo'): 1, (7, 0, 'lo'): 1,
        (7, 1, 'lo'): 1},
    blocks=[(0, 32, 48), (0, 80, 48), (0, 128, 48), (0, 176, 48), (0, 224, 32), (1, 32, 48), (1, 80, 48), (1, 128, 64),
        (1, 192, 64), (0, 0, 32), (1, 0, 32)],
    sub={(0, 0, 1): 16, (0, 32, 0): 16, (0, 80, 0): 16, (0, 128, 1): 16, (0, 176, 0): 16, (0, 224, 0): 16,
        (1, 0, 0): 16, (1, 32, 1): 16, (1, 80, 1): 16, (1, 192, 0): 32, (1, 192, 1): 16},
    pat={(0, 0, 0): ('p', 2, 2), (0, 0, 1): ('p', 2, 2), (0, 16, 1): ('p', 3, 2), (0, 32, 0): ('p', 0, 1),
        (0, 32, 1): ('p', 3, 0), (0, 64, 0): ('p', 0, 0), (0, 80, 0): ('p', 0, 1), (0, 80, 1): ('p', 0, 1),
        (0, 112, 0): ('p', 0, 0), (0, 128, 0): ('p', 3, 0), (0, 128, 1): ('p', 0, 0), (0, 160, 1): ('p', 3, 0),
        (0, 176, 0): ('p', 3, 2), (0, 176, 1): ('p', 0, 0), (0, 208, 0): ('p', 2, 2), (0, 224, 0): ('p', 3, 2),
        (0, 224, 1): ('p', 2, 1), (0, 240, 0): ('r', 0, 2, 0), (1, 0, 0): ('p', 2, 2), (1, 0, 1): ('p', 2, 2),
        (1, 16, 0): ('p', 0, 1), (1, 32, 0): ('p', 3, 2), (1, 32, 1): ('r', 3, 0, 2), (1, 64, 1): ('r', 2, 3, 0),
        (1, 80, 0): ('p', 0, 0), (1, 80, 1): ('p', 0, 0), (1, 112, 1): ('p', 3, 1), (1, 128, 0): ('p', 3, 0),
        (1, 128, 1): ('p', 2, 0), (1, 192, 0): ('p', 0, 2), (1, 192, 1): ('p', 0, 0), (1, 224, 0): ('r', 2, 0, 3),
        (1, 240, 1): ('p', 3, 1)},
)

ORDER = [
    ['b0>3', 'b0>1', 'L0K0p2', 'L0V0G1', 'L0K0p5', 'L0K1p1', 'L0K1p7', 'L0K0p4', 'L0V0p5', 'L0xg', 'L0Wq', 'L0K0p3',
     'L0K1G2', 'L0x1', 'L0x0', 'L0V1p0', 'L0V0p4', 'L0K0G0', 'L0V0G0', 'L0K1G1', 'L0K1p0', 'L0V1G1', 'L0K0G3', 'L0V1G2',
     'L0V1p1', 'L0Wo0', 'L0Wo1', 'L0V1G3', 'L0K1p6', 'L0V0G3', 'cvK0p5', 'cvK0p4', 'cvK0p2', 'cvV0p3', 'V0p3', 'K0p5',
     'cvK0p3 cvV0p5 cvWq0', 'Q0g', 'V0p5', 'Q0g>1', 'K0p2', 'cvV0p2', 'cvK1p4', 'V0p2', 'K0p4', 'K0p3', 'cvV0p4',
     'V0p4', 'Q0b1', 'Q0b0', 'S0p0lo T0p1lo', 'T1p0hi S0p0hi S0p1hi T0p0hi', 'K1p4', 'cvK1p2 T0p0lo', 'T1p3lo T1p0lo',
     'K1p2', 'cvV1p4', 'cvWo1', 'cvV1p2 cvWo0 S1p1hi', 'V1p4', 'V1p2', 'S1p7lo T1p7hi', 'T1p1lo T1p5hi', 'c1p5.192~',
     'c1p5.128~', 'T1p6lo T1p3hi T1p7lo', 'c1p3.80', 'S1p5lo T1p5lo pk1p5', 'st1p5~', 'c1p3.32', 'c1p5.0~', 'c1p5.32~',
     'P0_1.32 P0_1.80', 'c1p3.0', 'c1p5.80~', 'R0>1_1.112.1', 'U0>3_1.32.1', 'L0>3_1.80.1', 'U0>1_1.64.1',
     'T1p1hi pk1p3', 'R0>1_1.32.0', 'L0>3_1.80.0', 'st1p3', 'c1p3.192', 'c1p3.128', 'S0p7lo T0p1hi T1p6hi pw1p6 pw1p7',
     'P0_1.192', 'L0>3_1.192.0', 'P0_1.128', 'R0>1_1.128.0', 'U0>3_1.224.0', 'R0>1_1.240.1', 'L0>3_1.192.1',
     'T0p6lo T0p6hi T0p7lo P0_0.80', 'R0>1_1.128.1', 'L0>3_0.112.0', 'L0>3_0.80.1', 'T0p7hi P0_0.32', 'L0>3_0.80.0',
     'L0>3_0.64.0', 'R0>1_0.32.1', 'pw0p6 pw0p7 P0_0.224 P0_0.176', 'R0>1_0.224.1', 'L0>3_0.176.1', 'P0_0.128',
     'R0>1_0.160.1', 'R0>1_0.128.0', 'L0>3_0.128.1', 'pm3 pg0G3', 'R0>1_0.176.0', 'L0>3_0.32.0', 'a0_0.240.0_0 pm0',
     'a0_0.176.0_0', 'R0>1_0.208.0', 'pg0G0', 'P0_0.0 pg1G3', 'B0>3_0.240.0', 'pg1G0', 'R0>1_0.224.0', 'F0>3_0.176.0',
     'F0_0.176.0', 'F0_0.208.0', 'F0_0.224.0', 'F0_0.224.1', 'F0_0.128.0', 'F0_0.80.0', 'F0_0.240.0', 'F0_0.32.0',
     'a0_0.16.1_0 a0_0.224.0_0 P0_1.0', 'R0>1_0.16.1', 'a0_0.208.0_0', 'F0>3_0.224.0', 'a0_0.80.0_0', 'L0>3_0.208.0',
     'a0_0.32.0_0', 'a0_0.0.1_0 a0_0.0.0_0', 'L0>3_0.0.0', 'a0_1.0.0_0', 'a0_0.80.1_0', 'F0>1_0.80.1', 'R0>1_1.0.1',
     'F0>1_0.32.0', 'F0_0.64.0', 'F0_0.32.1', 'F0_0.0.0', 'F0_0.80.1', 'F0_0.16.1', 'F0_0.0.1', 'F0_0.128.1',
     'F0_1.0.0', 'a0_1.0.1_0', 'R0>1_1.0.0', 'L0>3_1.0.1', 'L0>3_1.16.0', 'L0>3_0.0.1', 'F0_1.0.1', 'F0_0.176.1',
     'F0_0.112.0', 'F0_1.32.0',
     '# V0p3 K0p5 V0p5 Q0g>1 K0p2 V0p2 K0p4 K0p3 V0p4 K1p4 K1p2 V1p4 V1p2 c1p5.192~ c1p5.128~ c1p3.80 st1p5~',
     'B0>1_1.32.1', 'R0>1_0.0.1', 'F0>3_0.16.1', 'a0_1.32.0_0', 'R0>1_0.0.0', 'L0>3_1.0.0', 'F0_1.32.1', 'F0_1.64.1',
     '# c1p3.32 c1p5.0~ c1p5.32~ c1p3.0 c1p5.80~ R0>1_1.112.1 U0>3_1.32.1 L0>3_1.80.1 U0>1_1.64.1 R0>1_1.32.0 '
     'L0>3_1.80.0 st1p3 c1p3.192 c1p3.128 L0>3_1.192.0 R0>1_1.128.0 U0>3_1.224.0 R0>1_1.240.1 L0>3_1.192.1 '
     'R0>1_1.128.1 L0>3_0.112.0 L0>3_0.80.1 L0>3_0.80.0 L0>3_0.64.0 R0>1_0.32.1 R0>1_0.224.1 L0>3_0.176.1 R0>1_0.160.1 '
     'R0>1_0.128.0 L0>3_0.128.1 R0>1_0.176.0 L0>3_0.32.0 R0>1_0.208.0 B0>3_0.240.0 R0>1_0.224.0 F0>3_0.176.0',
     'a0_1.128.1_0', 'F0>1_0.80.0', 'L0>3_1.128.1', 'F0_1.80.1', 'F0_1.128.1', 'F0_1.80.0',
     '# R0>1_0.16.1 F0>3_0.224.0 L0>3_0.208.0 L0>3_0.0.0 F0>1_0.80.1', 'a0_1.16.0_0', 'F0>1_1.16.0', 'F0>3_1.32.0',
     'F0_1.16.0', 'F0_1.128.0', 'F0_0.160.1',
     '# R0>1_1.0.1 F0>1_0.32.0 R0>1_1.0.0 L0>3_1.0.1 L0>3_1.16.0 L0>3_0.0.1 B0>1_1.32.1 F0>3_0.16.1 L0>3_1.0.0',
     'F0_1.192.1', 'F0_1.192.0', '# R0>1_0.0.1', 'F0_1.240.1', '# R0>1_0.0.0 L0>3_1.128.1', 'F0_1.112.1', 'F0_1.224.0'],
    ['b1>0', 'L1v1p0a', 'b1>2', 'L1v1p0', 'L1v0p0', 'L1k1G2', 'L1k0G0', 'L1Wq', 'L1v0p1', 'L1xg', 'L1v0G2', 'L1v1G2',
     'L1k1G0', 'L1k0G2', 'L1x1', 'L1x0', 'L1KVG2', 'L1k0G3', 'L1v1G3', 'L1k1G3', 'L1v0G3', 'L1v1p1', 'L1KVG0', 'L1Wo0',
     'L1k0G1', 'L1v0G1', 'L1Wo1', 'L1v1G1', 'L1k1G1', 'cvv1p0a', 'v1p0a', 'cvv1p0 cvv0p0', 'v0p0', 'cvk0p0 cvk0p1',
     'k0p0', 'k0p1', 'v1p0', 'cvk1p4', 'k1p4', 'cvWq1', 'Q1g', 'Q1g>2', 'cvv0p1', 'cvv0p4', 'cvk1p0', 'v0p4',
     'cvk1p1 cvk0p4', 'k0p4', 'cvv1p4', 'k1p0', 'v1p4', 'Q1b1', 'Q0g>2', 'k1p1', 'q1p3lo', 'q1p3hi', 'Q1b0', 'H0p5',
     'hs0p5', 'q1p5hi', 'h0p5', 'Z1G2', 'v0p1', 'cvv1p1', 'z1G2', 'H1p5 Z1G3', 'q1p5lo', 'z1G3', 'hs1p5', 'v1p1',
     'T0p2lo', 'Z1G0', 'z1G0', 'T0p3lo H1p6 cvWo2', 'h1p5', 'hs1p6', 'cvWo3', 'h1p6', 'P1_0.32 H1p7 P1_0.80', 'hs1p7',
     'R1>2_0.80.0', 'R1>2_0.32.0', 'R1>2_0.64.0', 'h1p7', 'T0p3hi H0p7', 'R1>2_0.80.1', 'R1>2_0.112.0', 'h0p7',
     'S0p2hi H0p6 T0p2hi P1_0.128', 'h0p6', 'hs0p7', 'R1>2_0.128.1', 'hs0p6', 'T1p2lo P1_0.176', 'R1>2_0.176.1',
     'a1_0.208.0_0', 'L1>0_0.208.0', 'P1_1.80 P1_1.32', 'U1>2_1.32.1', 'a1_0.128.0_1', 'R1>2_1.80.1',
     'a1_0.176.0_1 a1_1.112.1_0', 'L1>0_0.128.0', 'L1>0_0.176.0', 'a1_1.64.1_0', 'U1>2_1.64.1', 'R1>2_1.112.1',
     'T1p2hi H1p3 P1_0.224 Z1G1', 'a1_0.224.0_1', 'L1>0_0.224.0', 'R1>2_1.80.0', 'a1_0.224.1_1', 'L1>0_0.224.1',
     'pm1 a1_0.240.0_0 pw1p3', 'U1>0_0.240.0', 'pg1G1 pg0G1 P1_1.0', 'a1_0.32.1_1', 'L1>0_0.32.1', 'R1>2_1.16.0',
     'P1_1.192', 'R1>2_1.192.1', 'U1>2_1.224.0', 'P1_0.0 a1_0.0.0_0', 'a1_0.16.1_1', 'L1>0_0.0.0',
     'a1_0.0.1_0 a1_0.160.1_1', 'L1>0_0.16.1', 'a1_1.240.1_0', 'P1_1.128',
     '# v1p0a v0p0 k0p0 k0p1 v1p0 k1p4 Q1g>2 v0p4 k0p4 k1p0 v1p4 Q0g>2 k1p1 q1p3lo q1p3hi hs0p5 q1p5hi', 'a1_1.0.0_0',
     'L1>0_0.0.1', 'a1_1.128.0_0 a1_1.0.1_0', 'R1>2_1.240.1', 'a1_1.32.0_0', 'L1>0_1.0.0', 'R1>2_1.128.0', 'L1>0_1.0.1',
     '# h0p5 v0p1 z1G2 q1p5lo z1G3 hs1p5 v1p1 z1G0 h1p5 hs1p6 h1p6 hs1p7 R1>2_0.80.0 R1>2_0.32.0 R1>2_0.64.0 h1p7 '
     'R1>2_0.80.1 R1>2_0.112.0 h0p7 h0p6 hs0p7 R1>2_0.128.1 hs0p6 R1>2_0.176.1 L1>0_0.208.0 U1>2_1.32.1 R1>2_1.80.1 '
     'L1>0_0.128.0 L1>0_0.176.0 U1>2_1.64.1 R1>2_1.112.1 L1>0_0.224.0 L1>0_0.224.1',
     'a1_1.32.0_1', 'L1>0_1.32.0', 'F1_1.32.0', '# R1>2_1.80.0 U1>0_0.240.0 R1>2_1.16.0', 'a1_0.32.1_0', 'R1>2_1.192.0',
     'F1_0.32.1', '# L1>0_0.32.1', 'a1_1.128.1_1', 'L1>0_1.128.1', 'R1>2_0.32.1', 'a1_0.224.1_0', 'F1_0.224.1',
     'F1_1.128.1', 'a1_1.128.1_0 a1_0.160.1_0', 'R1>2_0.160.1', 'F1_0.160.1',
     '# R1>2_1.192.1 U1>2_1.224.0 L1>0_0.0.0 L1>0_0.16.1', 'a1_0.128.0_0', 'a1_1.128.0_1', 'R1>2_0.224.1',
     'R1>2_0.128.0', 'L1>0_1.128.0', 'F1_0.128.0', 'F1_1.128.0', 'F1_1.112.1', 'a1_0.176.0_0', 'L1>0_0.160.1',
     'F1_0.176.0', 'F1_1.64.1', 'F1_0.208.0', '# L1>0_0.0.1 R1>2_1.240.1 L1>0_1.0.0 R1>2_1.128.0 L1>0_1.0.1',
     'a1_0.224.0_0', 'R1>2_1.128.1', 'a1_1.192.0_0', 'F1_0.224.0', 'F1_1.192.0', 'a1_0.16.1_0', 'R1>2_0.224.0',
     'F1>0_1.192.0', 'R1>2_1.32.0', 'R1>2_0.16.1', 'F1_0.16.1', 'B1>0_1.224.0', 'F1_1.224.0', 'F1_1.240.1', 'F1_0.80.1',
     'F1_1.80.1', 'F1_1.0.1', 'F1_0.32.0', 'F1_1.80.0', 'F1_1.0.0',
     '# L1>0_1.32.0 R1>2_1.192.0 L1>0_1.128.1 R1>2_0.32.1 R1>2_0.160.1 R1>2_0.224.1 R1>2_0.128.0 L1>0_1.128.0 '
     'L1>0_0.160.1',
     'B1>2_1.32.1', 'R1>2_0.176.0', 'F1_1.32.1', 'F1_1.192.1', 'F1_0.0.1',
     '# R1>2_1.128.1 R1>2_0.224.0 F1>0_1.192.0 B1>0_1.224.0', 'F1_0.0.0', 'F1_0.176.1', '# R1>2_1.32.0 R1>2_0.16.1',
     'F1_0.112.0', 'F1_0.80.0', 'F1_0.240.0', 'F1_1.16.0', 'F1_0.64.0', '# B1>2_1.32.1', 'F1_0.128.1'],
    ['L2xg', 'L2Wq', 'L2x0', 'L2x1', 'L2Wo1', 'L2Wo0', 'L2KVG3', 'L2KVG0', 'L2KVG1', 'L2KVG2', 'r2>1', 'r2>3',
     'cvWq2 Q2g', 'Q2g>1', 'Q2g>3', 'Q2b0', 'q0p5hi', 'q0p5lo', 'q0p5h1', 'Q2b1', 'q1p5hi~', 'Q1g>3', 'Q3g>1', 'cvWo4',
     'q0p4hi', 'q1p5lo~', 'H0p4', 'q1p6h1', 'q0p4lo', 'cvWo5', 'q1p7h1', 'Z2G3', 'q0p7h1', 'q1p4lo', 'q1p4hi', 'Q0g>3',
     'Z2G0', 'q0p6h1', 'pw0p5', 'Z2G1', 'm2G1', 'z2G1', 'm2G3', 'z2G3', 'pw0p4 P2_0.176', 'L2>1_0.208.0',
     'L2>1_0.176.0', 'P2_0.128', 'L2>1_0.128.0', 'm2G0', 'z2G0', 'P2_0.224', 'U2>1_0.240.0', 'L2>1_0.224.1',
     'L2>1_0.160.1', 'Z2G2 P2_0.80', 'L2>1_0.224.0', 'a2_0.80.0_0', 'R2>3_0.80.0', 'P2_0.32 H1p4',
     'a2_0.32.0_0 a2_0.64.0_0', 'L2>1_0.32.1', 'R2>3_0.32.0', 'R2>3_0.64.0', 'pm2 pg0G2 P2_0.0', 'L2>1_0.0.0',
     'a2_0.80.1_0', 'R2>3_0.80.1', 'L2>1_0.16.1', 'a2_0.112.0_0 pw1p4 pg1G2', 'a2_0.128.1_0', 'L2>1_0.0.1',
     'R2>3_0.128.1', 'P2_1.0', 'L2>1_1.0.1', 'R2>3_0.112.0', 'L2>1_1.0.0', 'pw1p5', 'a2_0.176.1_0', 'R2>3_0.176.1',
     'P2_1.32', 'L2>1_1.32.0', 'a2_1.32.1_0', 'P2_1.128', 'U2>3_1.32.1', 'L2>1_1.128.1', 'P2_1.80 a2_1.80.1_0',
     'R2>3_1.80.1', 'L2>1_1.128.0', 'a2_1.64.1_0', 'B2>3_1.64.1', 'F2_1.64.1', 'F2_1.112.1',
     '# Q2g>1 Q2g>3 q0p5hi q0p5lo q0p5h1 q1p5hi~ Q1g>3 Q3g>1 q0p4hi q1p5lo~ q1p6h1 q0p4lo q1p7h1 q0p7h1 q1p4lo q1p4hi '
     'Q0g>3 q0p6h1 z2G1 z2G3 L2>1_0.208.0 L2>1_0.176.0 L2>1_0.128.0 z2G0 U2>1_0.240.0 L2>1_0.224.1 L2>1_0.160.1 '
     'L2>1_0.224.0 R2>3_0.80.0 L2>1_0.32.1 R2>3_0.32.0 R2>3_0.64.0 L2>1_0.0.0 R2>3_0.80.1 L2>1_0.16.1 L2>1_0.0.1',
     'a2_1.80.1_1', 'F2_1.80.1', '# R2>3_0.128.1 L2>1_1.0.1 R2>3_0.112.0 L2>1_1.0.0', 'a2_1.80.0_0', 'R2>3_1.80.0',
     'a2_1.112.1_0 a2_1.16.0_0 P2_1.192', 'R2>3_1.16.0', 'L2>1_1.112.1', 'B2>1_1.64.1', '# R2>3_0.176.1 L2>1_1.32.0',
     'a2_1.192.1_0', 'R2>3_1.192.1', '# U2>3_1.32.1', 'a2_1.192.0_1', 'L2>1_1.192.0', 'a2_1.224.0_0', 'B2>1_1.224.0',
     'F2_1.224.0', '# L2>1_1.128.1 R2>3_1.80.1', 'a2_1.240.1_0', 'R2>3_1.240.1', 'B2>3_1.224.0', 'L2>1_1.240.1',
     'R2>3_1.112.1', 'L2>1_1.80.1', 'F2_1.240.1', 'a2_1.80.0_1', 'L2>1_1.80.0', 'F2_1.80.0', 'F2_0.112.0',
     '# B2>3_1.64.1', 'a2_1.128.0_0', 'R2>3_1.128.0', 'F2_1.128.0', 'F2_1.192.1',
     '# L2>1_1.128.0 R2>3_1.80.0 R2>3_1.16.0 L2>1_1.112.1', 'a2_0.64.0_1 a2_1.192.0_0 a2_1.192.1_1', 'L2>1_1.192.1',
     'R2>3_1.192.0', 'F2_1.192.0', 'F2_0.64.0', '# B2>1_1.64.1', 'a2_0.176.1_1 a2_0.32.1_0', 'L2>1_0.176.1',
     'R2>3_0.32.1', 'a2_0.112.0_1', 'L2>1_0.112.0', 'F2_0.32.1', 'F2_0.176.1', 'F2_0.160.1', 'F2_0.128.1',
     '# R2>3_1.192.1 L2>1_1.192.0 B2>1_1.224.0 R2>3_1.240.1 B2>3_1.224.0 L2>1_1.240.1 R2>3_1.112.1',
     'a2_0.160.1_0 a2_0.224.1_0', 'F2>3_0.224.1', 'R2>3_0.160.1', 'F2_0.224.1', 'F2_0.80.1', '# L2>1_1.80.1',
     'a2_0.128.0_0', 'a2_0.128.1_1', 'B2>1_0.240.0', 'R2>3_0.128.0', 'L2>1_0.64.0', 'L2>1_0.128.1', 'F2_0.128.0',
     'F2_0.240.0', '# L2>1_1.80.0 R2>3_1.128.0 L2>1_1.192.1 R2>3_1.192.0', 'F2_0.80.0', '# R2>3_0.32.1', 'F2_1.128.1',
     'F2_0.32.0', '# L2>1_0.176.1 L2>1_0.112.0 F2>3_0.224.1 R2>3_0.160.1 B2>1_0.240.0', 'F2_0.224.0', 'F2_0.208.0',
     '# L2>1_0.64.0', 'F2_1.0.1', '# R2>3_0.128.0', 'F2_1.32.0', 'F2_1.16.0', '# L2>1_0.128.1', 'F2_0.16.1', 'F2_0.0.0',
     'F2_1.32.1', 'F2_0.0.1', 'F2_1.0.0', 'F2_0.176.0'],
    ['b3>0', 'L3Wo0.0', 'b3>2', 'L3Wo0.16', 'L3Wq', 'L3Wo1.64', 'L3Wo1.0', 'L3xg', 'L3x1', 'L3x0', 'L3Wo0.64', 'L3KVG1',
     'L3KVG0', 'L3KVG2', 'L3KVG3', 'cvWo6.0', 'Wo6.0', 'cvWo6.16', 'Wo6.16', 'cvWo7.64', 'Wo7.64', 'cvWq3', 'cvWo7.0',
     'Wo7.0', 'Q3g', 'Q3g>2', 'Q3b1', 'q1p7lo', 'q1p6h1~', 'q1p7hi', 'q1p7h1~', 'cvWo6.64', 'q1p6lo', 'Q3b0', 'q0p7h1~',
     'Wo6.64', 'q1p6hi', 'S0p5hi T0p5hi', 'q0p7lo', 'c0p5.128', 'S0p5lo T0p5lo', 'q0p6lo', 'q0p6hi', 'q0p6h1~', 'pk0p5',
     'st0p5', 'Z3G1', 'z3G1', 'S0p4hi', 'T0p4hi', 'c0p4.128', 'c0p4.176', 'S0p4lo pk0p4', 'st0p4', 'q0p7hi', 'c0p5.0',
     'T0p4lo', 'c0p4.224', 'c0p4.80', 'c0p4.0', 'c0p4.32', 'Z3G2', 'z3G2', 'Z3G3 S1p4lo', 'Z3G0', 'T1p4lo', 'c1p4.32',
     'c1p4.80', 'T1p4hi', 'pk1p4', 'st1p4', 'st1p5', 'c1p4.0', 'c1p5.0', 'm3G3', 'c1p5.32', 'c1p4.128', 'c1p5.128',
     'c1p5.80', 'z3G3', 'm3G0', 'z3G0', 'c1p5.192', 'R3>0_0.80.0', 'L3>2_1.80.1', 'c1p4.192',
     '# Wo6.0 Wo6.16 Wo7.64 Wo7.0 Q3g>2 q1p7lo q1p6h1~ q1p7hi q1p7h1~ q1p6lo q0p7h1~ Wo6.64 q1p6hi q0p7lo c0p5.128 '
     'q0p6lo q0p6hi q0p6h1~ st0p5 z3G1 c0p4.128 c0p4.176 st0p4 c0p5.0 c0p4.224 c0p4.80 c0p4.0 c0p4.32 z3G2 c1p4.32 '
     'c1p4.80 st1p4 st1p5 c1p4.0',
     'R3>0_0.32.0', '# q0p7hi c1p5.0 c1p5.32', 'U3>2_1.224.0', 'R3>0_0.64.0', 'L3>2_1.192.0', '# c1p4.128 z3G3',
     'R3>0_0.80.1', 'L3>2_1.80.0', '# c1p5.128', 'R3>0_0.128.1', 'F3_0.112.0', '# c1p5.80 c1p5.192', 'R3>0_0.176.1',
     'L3>2_0.112.0', 'L3>2_1.192.1', 'F3_0.80.1', 'F3_0.80.0', 'a3_1.32.1_0', 'R3>0_0.112.0', 'B3>0_1.32.1',
     'L3>2_0.64.0', 'F3_1.32.1', 'F3_0.64.0', 'F3_1.80.1',
     '# z3G0 R3>0_0.80.0 L3>2_1.80.1 c1p4.192 R3>0_0.32.0 U3>2_1.224.0 R3>0_0.64.0', 'B3>0_1.64.1', 'R3>0_1.80.1',
     'F3_1.64.1', 'L3>2_0.176.1', 'F3_0.176.1', '# L3>2_1.192.0 R3>0_0.80.1', 'L3>2_0.128.1', 'L3>2_0.80.1',
     'F3_0.128.1', 'R3>0_1.80.0', 'F3_1.80.0', 'F3_0.32.0', '# L3>2_1.80.0 R3>0_0.128.1 L3>2_0.112.0', 'B3>2_0.240.0',
     'R3>0_1.16.0', 'F3_0.240.0', '# R3>0_0.176.1', 'R3>0_1.192.1', 'L3>2_0.80.0', 'F3_1.192.1', 'F3_0.176.0',
     'F3>0_1.240.1', 'F3_1.240.1', 'F3_0.224.0', 'F3_0.208.0', 'F3_1.224.0',
     '# L3>2_1.192.1 R3>0_0.112.0 B3>0_1.32.1 L3>2_0.64.0 B3>0_1.64.1 L3>2_0.176.1', 'F3>0_1.112.1', 'L3>2_0.32.0',
     'F3>2_0.208.0', 'F3_1.112.1', 'F3_0.0.0', '# R3>0_1.80.1', 'F3>2_1.0.1', 'F3_1.0.1', '# L3>2_0.128.1',
     'L3>2_1.16.0', 'F3>2_0.0.0', 'F3_1.16.0', '# R3>0_1.80.0', 'F3>2_0.0.1', 'F3_1.128.0', 'F3_0.0.1', 'F3_0.16.1',
     '# L3>2_0.80.1 B3>2_0.240.0 R3>0_1.16.0', 'F3>2_1.0.0', 'F3_1.192.0', 'F3_1.0.0',
     '# R3>0_1.192.1 L3>2_0.80.0 F3>0_1.240.1 F3>0_1.112.1 L3>2_0.32.0 F3>2_0.208.0', 'F3_0.32.1',
     '# F3>2_1.0.1 L3>2_1.16.0', 'F3_1.128.1', 'F3_0.224.1', '# F3>2_0.0.0', 'F3_0.160.1', '# F3>2_0.0.1', 'F3_1.32.0',
     '# F3>2_1.0.0', 'F3_0.128.0'],
]

LAYOUT = [(1, 156), (2, 37), (3, 86), (0, None), (1, None), (2, None), (3, None)]


def pallas_dist_sparse_attn_localglobal_htp_kvseq_b2_sq256_skv256_hq4_dh64_kernel(x, Wq, K_ext, V_ext, Wo):
    return make_kernel(make_tasks(CFG), ORDER, CFG['w'], LAYOUT)(x, Wq, K_ext, V_ext, Wo)
```
